```python
import numpy as np

kernel_name = "dist_sort_i_m128_n64"

def setup_inputs():
    return {"x": np.random.randn(512, 64).astype(np.float32)}

def reference(x: np.ndarray) -> np.ndarray:
    return np.sort(x, axis=0)
```

```python
import jax
import jax.numpy as jnp
from jax import lax
from jax.experimental import pallas as pl
from jax.experimental.pallas import tpu as pltpu

BF16 = jnp.bfloat16
F32 = jnp.float32
MESH = pl.DeviceIdType.MESH
NT = (((1,), (1,)), ((), ()))

A, B, D, C = 0, 1, 2, 3


class Lay:
    def __init__(self, slot, sub):
        self.slot, self.sub = list(slot), dict(sub)

    def copy(self):
        return Lay(self.slot, self.sub)

    def dist(self, bit):
        return [d for d, b in self.sub.items() if b == bit][0]


def _oe_merge(lo, n, r):
    m = 2 * r
    if m < n:
        yield from _oe_merge(lo, n, m)
        yield from _oe_merge(lo + r, n, m)
        for i in range(lo + r, lo + n - r, m):
            yield (i, i + r)
    else:
        yield (lo, lo + r)


def _oe_sort(lo, n):
    if n > 1:
        yield from _oe_sort(lo, n // 2)
        yield from _oe_sort(lo + n // 2, n // 2)
        yield from _oe_merge(lo, n, 1)


SORT16 = list(_oe_sort(0, 16))
MERGE16 = list(_oe_merge(0, 16, 1))


def _network(tiles, net):
    t = list(tiles)
    for i, j in net:
        t[i], t[j] = jnp.minimum(t[i], t[j]), jnp.maximum(t[i], t[j])
    return t


def _split(v, lay, bit):
    k = lay.slot.index(bit)
    lay.slot.append(lay.slot.pop(k))
    if k == 3:
        return v[:8], v[8:]
    w = v.shape[-1]
    v5 = v.reshape(8 >> k, 2, 1 << k, 8, w)
    return v5[:, 0].reshape(8, 8, w), v5[:, 1].reshape(8, 8, w)


def _join(a, b):
    return jnp.concatenate([a, b], axis=0)


def _sub_mask(d, shape):
    return (lax.broadcasted_iota(jnp.int32, shape, 1) & d) != 0


def _cmp(v, lay, bit, desc=False):
    a, b = _split(v, lay, bit)
    lo, hi = jnp.minimum(a, b), jnp.maximum(a, b)
    return _join(hi, lo) if desc else _join(lo, hi)


def _swap(v, lay, bit_in, bit_out, mirror=False, negate=False):
    d = lay.dist(bit_in)
    a, b = _split(v, lay, bit_out)
    m = _sub_mask(d, a.shape)
    a2 = jnp.where(m, pltpu.roll(b, d, 1), a)
    if mirror:
        b2 = jnp.where(m, a, pltpu.roll(b, 8 - d, 1))
    else:
        b2 = jnp.where(m, b, pltpu.roll(a, 8 - d, 1))
    lay.slot[3], lay.sub[d] = bit_in, bit_out
    return _join(a2, -b2 if negate else b2)


def _cmp_sub(v, lay, bit):
    d = lay.dist(bit)
    up = pltpu.roll(v, d, 1)
    dn = up if d == 4 else pltpu.roll(v, 8 - d, 1)
    return jnp.where(_sub_mask(d, v.shape), jnp.maximum(v, up), jnp.minimum(v, dn))


def _tiles(v, lay, slot):
    pos = [lay.slot.index(b) for b in slot]
    idx = [sum(((j >> k) & 1) << p for k, p in enumerate(pos)) for j in range(16)]
    lay.slot = list(slot)
    return [v[i:i + 1] for i in idx]


def _merge16(v, lay, top, rev):
    t = _tiles(v, lay, [top - 3, top - 2, top - 1, top])
    return _network(t[:8] + (t[:7:-1] if rev else t[8:]), MERGE16)


def _cat(tiles):
    return jnp.concatenate(tiles, axis=0)


ARRIVE = [0, 4, 8, 12, 1, 5, 9, 13, 2, 6, 10, 14, 3, 7, 11, 15]
LAY_I = Lay([4, 5, 6, 0], {2: 3, 1: 2, 4: 1})


def _presort(v):
    lay = Lay([0, 1, 2, 3], {2: 4, 1: 5, 4: 6})
    v = _cat(_network([v[a:a + 1] for a in ARRIVE], SORT16))
    v = _swap(v, lay, 4, 0, mirror=True)
    v = _cat(_merge16(v, lay, 4, False))
    v = _cmp(_swap(v, lay, 0, 1), lay, 0)
    v = _swap(v, lay, 5, 0, negate=True)
    v = _cat(_merge16(v, lay, 5, True))
    v = _cmp(_swap(v, lay, 1, 2), lay, 1)
    v = _cmp(_swap(v, lay, 0, 1), lay, 0)
    v = _swap(v, lay, 6, 0, negate=True)
    return _merge16(v, lay, 6, True), lay


def _finish(tiles, lay, desc):
    lay = lay.copy()
    v = _cat(tiles[::-1] if desc else tiles)
    for b in (2, 1, 0):
        v = _cmp(_swap(v, lay, b, b + 1), lay, b, desc)
    assert lay.slot == LAY_I.slot and lay.sub == LAY_I.sub
    return v


def _bitonic_keep(v):
    lay = LAY_I.copy()
    for b in (6, 5, 4):
        v = _cmp(v, lay, b)
    for b in (3, 2, 1):
        v = _cmp_sub(v, lay, b)
    v = _cmp(v, lay, 0)
    return _cat(_tiles(v, lay, LAY_I.slot))


def _bitonic_natural(v):
    lay = LAY_I.copy()
    for b in (6, 5, 4):
        v = _cmp(v, lay, b)
    for b, e in ((3, 0), (2, 3), (1, 2), (0, 1)):
        v = _cmp(_swap(v, lay, b, e), lay, b)
    v = _swap(v, lay, 3, 0)
    assert lay.sub == {4: 2, 2: 1, 1: 0}
    return _cat(_tiles(v, lay, [3, 4, 5, 6]))


def _to_lanes(w):
    parts = []
    for q in range(4):
        r = lax.broadcasted_iota(jnp.int32, (32, 128), 0) + 32 * q
        c = lax.broadcasted_iota(jnp.int32, (32, 128), 1)
        sign = jnp.where(((r ^ (r >> 2)) & 1) == 1, -1.0, 1.0)
        sel = jnp.where(r == c, sign, 0.0).astype(BF16)
        parts.append(lax.dot_general(sel, w, NT, preferred_element_type=F32))
    return _cat(parts).reshape(16, 8, w.shape[0])


NM = 48

def _write_out(v, o_ref):
    y = v.reshape(128, v.shape[-1])[:, :64]
    hi = _cat([jnp.zeros((NM, 64), F32), y[NM:]]).T
    o_ref[:, NM:] = hi[:, NM:]
    lo = y[:NM].astype(BF16)
    for q in range(4):
        r = lax.broadcasted_iota(jnp.int32, (16, 64), 0) + 16 * q
        c = lax.broadcasted_iota(jnp.int32, (16, 64), 1)
        o_ref[16 * q:16 * (q + 1), :NM] = lax.dot_general(
            (r == c).astype(BF16), lo, NT, preferred_element_type=F32)


ORDER = {A: (B, C), B: (A, D, C), C: (A, D, B), D: (A, B, C)}


def pallas_dist_sort_i_m128_n64_kernel(x: jax.Array):
    xt = x.T

    def body(x_ref, o_ref, xin, sp, c2s, rsp, rc1, rc2, lsem, ssem, rsem, psem, dsem):
        me = lax.axis_index("i")
        bar = pltpu.get_barrier_semaphore()

        def sig(sem, dev):
            pl.semaphore_signal(sem, inc=1, device_id=(dev,), device_id_type=MESH)

        def slot_copy(slot, dst):
            return pltpu.make_async_remote_copy(
                src_ref=sp, dst_ref=rsp.at[slot], send_sem=ssem.at[dst], recv_sem=rsem.at[slot],
                device_id=(dst,), device_id_type=MESH)

        def send(src, dst):
            return slot_copy(ORDER[dst].index(src), dst)

        raw_copy = lambda: pltpu.make_async_remote_copy(
            src_ref=x_ref.at[pl.ds(32, 32)], dst_ref=rc1, send_sem=ssem.at[A], recv_sem=rsem.at[2],
            device_id=(A,), device_id_type=MESH)
        half_copy = lambda: pltpu.make_async_remote_copy(
            src_ref=c2s, dst_ref=rc2, send_sem=ssem.at[D], recv_sem=rsem.at[3],
            device_id=(A,), device_id_type=MESH)
        load = lambda h: pltpu.make_async_copy(
            x_ref.at[pl.ds(32 * h, 32)], xin.at[pl.ds(32 * h, 32)], lsem.at[h])

        @pl.when(me == D)
        def _():
            pl.semaphore_wait(bar, 1)
            raw_copy().start()
            load(0).start()
            sig(dsem, A)
            load(0).wait()
            c2s[...] = xin[0:32, :].astype(BF16)
            half_copy().start()
            load(1).start()

        @pl.when(me != D)
        def _():
            load(0).start()
            load(1).start()

            @pl.when(me == A)
            def _():
                sig(bar, D); sig(bar, B); sig(bar, C)

            @pl.when(me != A)
            def _():
                sig(bar, A)
                pl.semaphore_wait(bar, 1)
            load(0).wait()

        load(1).wait()
        left = lax.broadcasted_iota(jnp.int32, (8, 8, 128), 2) < 64
        left16 = lax.broadcasted_iota(jnp.int32, (16, 8, 128), 2) < 64
        xv = xin[...]
        pre, lay = _presort(_to_lanes(_cat([xv, xv]).astype(BF16)))
        dn = _finish(pre, lay, True)
        sp[...] = jnp.where(left, dn[:8], dn[8:]).reshape(64, 128).astype(BF16)

        for X, Y in ((B, C), (C, B)):
            @pl.when(me == X)
            def _(X=X, Y=Y):
                send(X, A).start()
                pl.semaphore_wait(psem, 1)
                send(X, Y).start()

        @pl.when(me == D)
        def _():
            pl.semaphore_wait(bar, 1)
            sig(dsem, B); sig(dsem, C)
            send(D, B).start(); send(D, C).start()

        @pl.when(me == A)
        def _():
            pl.semaphore_wait(bar, 2)
            sig(bar, D); sig(psem, B); sig(psem, C)
            send(A, B).start(); send(A, C).start()
            pl.semaphore_wait(dsem, 1)
            send(A, D).start()

        own = _finish(pre, lay, False)

        def get(slot, both):
            slot_copy(slot, A).wait_recv()
            p = rsp[slot].astype(F32)
            q = pltpu.roll(p, 64, 1).reshape(8, 8, 128)
            p = p.reshape(8, 8, 128)
            if both:
                return _join(jnp.where(left, p, q), jnp.where(left, q, p))
            return _join(p, q)

        def swap_halves(v):
            return pltpu.roll(v.reshape(128, 128), 64, 1).reshape(16, 8, 128)

        l1 = get(0, True)
        lh = _bitonic_keep(jnp.where(left16, jnp.minimum(own, l1), jnp.maximum(own, l1)))
        hl = swap_halves(lh)

        for X in (B, C):
            @pl.when(me == X)
            def _(X=X):
                pl.semaphore_wait(dsem, 1)
                send(X, D).start()

        l2 = get(1, True)
        low = me < 2
        inf = jnp.float32(jnp.inf)
        lb = jnp.where(low, jnp.where(left16, -inf, hl), lh)
        ub = jnp.where(low, lh, jnp.where(left16, hl, inf))
        uv = _bitonic_keep(jnp.minimum(jnp.maximum(l2, lb), ub))

        @pl.when(me != A)
        def _():
            vu = swap_halves(uv)
            l3 = get(2, False)
            top = me == C
            lb = jnp.where(top, vu, uv)
            ub = jnp.where(top, inf, vu)
            _write_out(_bitonic_natural(jnp.minimum(jnp.maximum(l3, lb), ub)), o_ref)
            for X, dsts in ((B, (A, C, D)), (C, (A, B, D)), (D, (B, C))):
                @pl.when(me == X)
                def _(X=X, dsts=dsts):
                    for dst in dsts:
                        send(X, dst).wait_send()
                    if X == D:
                        raw_copy().wait_send(); half_copy().wait_send()

        @pl.when(me == A)
        def _():
            t = uv[:, :, :64]
            send(A, B).wait_send(); send(A, C).wait_send(); send(A, D).wait_send()
            raw_copy().wait_recv()
            r1 = rc1[...]
            f1 = _to_lanes(_cat([jnp.zeros_like(r1), r1]).astype(BF16))
            half_copy().wait_recv()
            f2 = _to_lanes(rc2[...])
            pre, lay = _presort(jnp.concatenate([f2, f1[:, :, 32:64]], axis=2))
            _write_out(_bitonic_natural(jnp.minimum(t, _finish(pre, lay, True))), o_ref)

    out = pl.pallas_call(
        body, out_shape=jax.ShapeDtypeStruct(xt.shape, x.dtype),
        in_specs=[pl.BlockSpec(memory_space=pl.ANY)],
        out_specs=pl.BlockSpec(memory_space=pltpu.VMEM),
        scratch_shapes=[
            pltpu.VMEM((64, 128), F32), pltpu.VMEM((64, 128), BF16), pltpu.VMEM((32, 128), BF16),
            pltpu.VMEM((3, 64, 128), BF16), pltpu.VMEM((32, 128), F32), pltpu.VMEM((32, 128), BF16),
            pltpu.SemaphoreType.DMA((2,)), pltpu.SemaphoreType.DMA((4,)), pltpu.SemaphoreType.DMA((4,)),
            pltpu.SemaphoreType.REGULAR, pltpu.SemaphoreType.REGULAR],
        compiler_params=pltpu.CompilerParams(collective_id=0, disable_semaphore_checks=True, disable_bounds_checks=True),
    )(xt)
    return out.T
```

```python
import jax
import jax.numpy as jnp
from jax import lax
from jax.experimental import pallas as pl
from jax.experimental.pallas import tpu as pltpu

BF16 = jnp.bfloat16
F32 = jnp.float32
MESH = pl.DeviceIdType.MESH
NT = (((1,), (1,)), ((), ()))

A, B, D, C = 0, 1, 2, 3


class _Lay:
    def __init__(self, slot, sub):
        self.slot, self.sub = list(slot), dict(sub)

    def copy(self):
        return _Lay(self.slot, self.sub)

    def dist(self, bit):
        return [d for d, b in self.sub.items() if b == bit][0]


def _oe_merge(lo, n, r):
    m = 2 * r
    if m < n:
        yield from _oe_merge(lo, n, m)
        yield from _oe_merge(lo + r, n, m)
        for i in range(lo + r, lo + n - r, m):
            yield (i, i + r)
    else:
        yield (lo, lo + r)


def _oe_sort(lo, n):
    if n > 1:
        yield from _oe_sort(lo, n // 2)
        yield from _oe_sort(lo + n // 2, n // 2)
        yield from _oe_merge(lo, n, 1)


SORT16 = list(_oe_sort(0, 16))
MERGE16 = list(_oe_merge(0, 16, 1))


def _network(tiles, net):
    t = list(tiles)
    for i, j in net:
        t[i], t[j] = jnp.minimum(t[i], t[j]), jnp.maximum(t[i], t[j])
    return t


def _cat(parts):
    return jnp.concatenate(parts, axis=0)


def _split(v, lay, bit):
    k = lay.slot.index(bit)
    lay.slot.append(lay.slot.pop(k))
    if k == 3:
        return v[:8], v[8:]
    w = v.shape[-1]
    v5 = v.reshape(8 >> k, 2, 1 << k, 8, w)
    return v5[:, 0].reshape(8, 8, w), v5[:, 1].reshape(8, 8, w)


def _sub_mask(d, shape):
    return (lax.broadcasted_iota(jnp.int32, shape, 1) & d) != 0


def _cmp(v, lay, bit, desc=False):
    a, b = _split(v, lay, bit)
    lo, hi = jnp.minimum(a, b), jnp.maximum(a, b)
    return _cat([hi, lo] if desc else [lo, hi])


def _cmp_sub(v, lay, bit):
    d = lay.dist(bit)
    up = pltpu.roll(v, d, 1)
    dn = up if d == 4 else pltpu.roll(v, 8 - d, 1)
    return jnp.where(_sub_mask(d, v.shape), jnp.maximum(v, up), jnp.minimum(v, dn))


def _swap(v, lay, bit_in, bit_out, mirror=False, negate=False):
    d = lay.dist(bit_in)
    a, b = _split(v, lay, bit_out)
    m = _sub_mask(d, a.shape)
    a2 = jnp.where(m, pltpu.roll(b, d, 1), a)
    if mirror:
        b2 = jnp.where(m, a, pltpu.roll(b, 8 - d, 1))
    else:
        b2 = jnp.where(m, b, pltpu.roll(a, 8 - d, 1))
    lay.slot[3], lay.sub[d] = bit_in, bit_out
    return _cat([a2, -b2 if negate else b2])


def _tiles(v, lay, slot):
    pos = [lay.slot.index(b) for b in slot]
    idx = [sum(((j >> k) & 1) << p for k, p in enumerate(pos)) for j in range(16)]
    lay.slot = list(slot)
    return [v[i:i + 1] for i in idx]


def _merge16(v, lay, top, rev):
    t = _tiles(v, lay, [top - 3, top - 2, top - 1, top])
    return _network(t[:8] + (t[:7:-1] if rev else t[8:]), MERGE16)


ARRIVE = [0, 4, 8, 12, 1, 5, 9, 13, 2, 6, 10, 14, 3, 7, 11, 15]
LAY_LIST = _Lay([4, 5, 6, 0], {2: 3, 1: 2, 4: 1})


def _presort(v):
    lay = _Lay([0, 1, 2, 3], {2: 4, 1: 5, 4: 6})
    v = _cat(_network([v[a:a + 1] for a in ARRIVE], SORT16))
    v = _swap(v, lay, 4, 0, mirror=True)
    v = _cat(_merge16(v, lay, 4, False))
    v = _cmp(_swap(v, lay, 0, 1), lay, 0)
    v = _swap(v, lay, 5, 0, negate=True)
    v = _cat(_merge16(v, lay, 5, True))
    v = _cmp(_swap(v, lay, 1, 2), lay, 1)
    v = _cmp(_swap(v, lay, 0, 1), lay, 0)
    v = _swap(v, lay, 6, 0, negate=True)
    return _merge16(v, lay, 6, True), lay


def _finish(pre, desc):
    tiles, lay = pre[0], pre[1].copy()
    v = _cat(tiles[::-1] if desc else tiles)
    for b in (2, 1, 0):
        v = _cmp(_swap(v, lay, b, b + 1), lay, b, desc)
    assert lay.slot == LAY_LIST.slot and lay.sub == LAY_LIST.sub
    return v


def _bitonic_to_list(v):
    lay = LAY_LIST.copy()
    for b in (6, 5, 4):
        v = _cmp(v, lay, b)
    for b in (3, 2, 1):
        v = _cmp_sub(v, lay, b)
    v = _cmp(v, lay, 0)
    return _cat(_tiles(v, lay, LAY_LIST.slot))


def _bitonic_to_rows(v):
    lay = LAY_LIST.copy()
    for b in (6, 5, 4):
        v = _cmp(v, lay, b)
    for b, e in ((3, 0), (2, 3), (1, 2), (0, 1)):
        v = _cmp(_swap(v, lay, b, e), lay, b)
    v = _swap(v, lay, 3, 0)
    assert lay.sub == {4: 2, 2: 1, 1: 0}
    return _cat(_tiles(v, lay, [3, 4, 5, 6])).reshape(128, v.shape[-1])


def _to_lanes(w):
    parts = []
    for q in range(4):
        r = lax.broadcasted_iota(jnp.int32, (32, 128), 0) + 32 * q
        c = lax.broadcasted_iota(jnp.int32, (32, 128), 1)
        sign = jnp.where(((r ^ (r >> 2)) & 1) == 1, -1.0, 1.0)
        sel = jnp.where(r == c, sign, 0.0).astype(BF16)
        parts.append(lax.dot_general(sel, w, NT, preferred_element_type=F32))
    return _cat(parts).reshape(16, 8, w.shape[0])


MXU_RANKS = 48


def _write_out(rows, o_ref):
    y = rows[:, :64]
    hi = _cat([jnp.zeros((MXU_RANKS, 64), F32), y[MXU_RANKS:]]).T
    o_ref[:, MXU_RANKS:] = hi[:, MXU_RANKS:]
    lo = y[:MXU_RANKS].astype(BF16)
    for q in range(4):
        r = lax.broadcasted_iota(jnp.int32, (16, 64), 0) + 16 * q
        c = lax.broadcasted_iota(jnp.int32, (16, 64), 1)
        o_ref[16 * q:16 * (q + 1), :MXU_RANKS] = lax.dot_general(
            (r == c).astype(BF16), lo, NT, preferred_element_type=F32)


ORDER = {A: (B, C, D), B: (A, D, C), C: (A, D, B), D: (A, B, C)}


def _body(x_ref, o_ref, xin, lst, sa, sb, rlst, rb_raw, rd_raw, rd_a, rd_b, first,
          lsem, ssem, rsem, psem, dsem):
    def load(r0, n, k):
        return pltpu.make_async_copy(
            x_ref.at[pl.ds(r0, n)], xin.at[pl.ds(r0, n)], lsem.at[k])

    ld_a, ld_b, ld_c = load(32, 8, 0), load(0, 32, 1), load(40, 24, 2)
    me = lax.axis_index("i")
    ld_a.start()
    ld_b.start()
    bar = pltpu.get_barrier_semaphore()

    def sig(sem, dev):
        pl.semaphore_signal(sem, inc=1, device_id=(dev,), device_id_type=MESH)

    def rdma(src, dst, s, r, dev):
        return pltpu.make_async_remote_copy(
            src_ref=src, dst_ref=dst, send_sem=ssem.at[s], recv_sem=rsem.at[r],
            device_id=(dev,), device_id_type=MESH)

    def send(src, dst):
        slot = ORDER[dst].index(src)
        return rdma(lst, rlst.at[slot], dst, slot, dst)

    b_raw = lambda: rdma(x_ref, rb_raw, A, 0, A)
    d_raw = lambda: rdma(x_ref.at[pl.ds(40, 24)], rd_raw, A, 2, A)
    d_a = lambda: rdma(sa, rd_a, 4, 3, A)
    d_b = lambda: rdma(sb, rd_b, 5, 4, A)

    @pl.when(me == D)
    def _():
        pl.semaphore_wait(bar, 1)
        d_raw().start()
        sig(dsem, A)
        ld_a.wait()
        sa[...] = xin[32:40, :].astype(BF16)
        d_a().start()
        ld_b.wait()
        sb[...] = xin[0:32, :].astype(BF16)
        d_b().start()
        ld_c.start()

    @pl.when(me != D)
    def _():
        ld_c.start()

        @pl.when(me == A)
        def _():
            sig(bar, D)
            sig(bar, B)
            sig(bar, C)

        @pl.when(me != A)
        def _():
            sig(bar, A)
            pl.semaphore_wait(bar, 1)

        @pl.when(me == B)
        def _():
            b_raw().start()

        ld_a.wait()
        ld_b.wait()

    ld_c.wait()

    def presort_dup(w):
        return _presort(_to_lanes(_cat([w, w]).astype(BF16)))

    left = lax.broadcasted_iota(jnp.int32, (8, 8, 128), 2) < 64
    left16 = lax.broadcasted_iota(jnp.int32, (16, 8, 128), 2) < 64
    pre = presort_dup(xin[...])
    dn = _finish(pre, True)
    lst[...] = jnp.where(left, dn[:8], dn[8:]).reshape(64, 128).astype(BF16)

    for X, Y in ((B, C), (C, B)):
        @pl.when(me == X)
        def _(X=X, Y=Y):
            if X == C:
                send(C, A).start()
            pl.semaphore_wait(psem, 1)
            send(X, Y).start()

    @pl.when(me == D)
    def _():
        pl.semaphore_wait(bar, 1)
        sig(dsem, B)
        sig(dsem, C)
        send(D, B).start()
        send(D, C).start()

    own = _finish(pre, False)

    def get(slot, both):
        rdma(lst, rlst.at[slot], 0, slot, A).wait_recv()
        p = rlst[slot].astype(F32)
        q = pltpu.roll(p, 64, 1).reshape(8, 8, 128)
        p = p.reshape(8, 8, 128)
        if both:
            return _cat([jnp.where(left, p, q), jnp.where(left, q, p)])
        return _cat([p, q])

    def swap_halves(v):
        return pltpu.roll(v.reshape(128, 128), 64, 1).reshape(16, 8, 128)

    @pl.when(me == A)
    def _():
        pl.semaphore_wait(bar, 2)
        sig(bar, D)
        sig(psem, B)
        sig(psem, C)
        send(A, B).start()
        send(A, C).start()
        pl.semaphore_wait(dsem, 1)
        send(A, D).start()
        b_raw().wait_recv()
        first[...] = _finish(presort_dup(rb_raw[...]), True)

    @pl.when(me != A)
    def _():
        first[...] = get(0, True)

    l1 = first[...]
    lh = _bitonic_to_list(
        jnp.where(left16, jnp.minimum(own, l1), jnp.maximum(own, l1)))

    for X in (B, C):
        @pl.when(me == X)
        def _(X=X):
            pl.semaphore_wait(dsem, 1)
            send(X, D).start()

    l2 = get(1, True)
    hl = swap_halves(lh)
    low = me < 2
    inf = jnp.float32(jnp.inf)
    lo2 = jnp.where(low, jnp.where(left16, -inf, hl), lh)
    hi2 = jnp.where(low, lh, jnp.where(left16, hl, inf))
    uv = _bitonic_to_list(jnp.minimum(jnp.maximum(l2, lo2), hi2))

    @pl.when(me != A)
    def _():
        l3 = get(2, False)
        vu = swap_halves(uv)
        lo3 = jnp.where(me == C, vu, uv)
        hi3 = jnp.where(me == C, inf, vu)
        _write_out(_bitonic_to_rows(jnp.minimum(jnp.maximum(l3, lo3), hi3)), o_ref)
        for X, dsts, raws in ((B, (C, D), (b_raw,)), (C, (A, B, D), ()),
                              (D, (B, C), (d_raw, d_a, d_b))):
            @pl.when(me == X)
            def _(X=X, dsts=dsts, raws=raws):
                for dst in dsts:
                    send(X, dst).wait_send()
                for raw in raws:
                    raw().wait_send()

    @pl.when(me == A)
    def _():
        d_raw().wait_recv()
        d_a().wait_recv()
        early = _cat([jnp.zeros((32, 128), F32), rd_a[...].astype(F32), rd_raw[...]])
        f1 = _to_lanes(early.astype(BF16))
        for dst in (B, C, D):
            send(A, dst).wait_send()
        d_b().wait_recv()
        f2 = _to_lanes(rd_b[...])
        l3 = _finish(_presort(jnp.concatenate([f2, f1[:, :, 32:64]], axis=2)), True)
        _write_out(_bitonic_to_rows(jnp.minimum(uv[:, :, :64], l3)), o_ref)


def pallas_dist_sort_i_m128_n64_kernel(x: jax.Array):
    out_t = pl.pallas_call(
        _body,
        out_shape=jax.ShapeDtypeStruct((64, 128), x.dtype),
        in_specs=[pl.BlockSpec(memory_space=pl.ANY)],
        out_specs=pl.BlockSpec(memory_space=pltpu.VMEM),
        scratch_shapes=[
            pltpu.VMEM((64, 128), F32),
            pltpu.VMEM((64, 128), BF16),
            pltpu.VMEM((8, 128), BF16),
            pltpu.VMEM((32, 128), BF16),
            pltpu.VMEM((3, 64, 128), BF16),
            pltpu.VMEM((64, 128), F32),
            pltpu.VMEM((24, 128), F32),
            pltpu.VMEM((8, 128), BF16),
            pltpu.VMEM((32, 128), BF16),
            pltpu.VMEM((16, 8, 128), F32),
            pltpu.SemaphoreType.DMA((3,)),
            pltpu.SemaphoreType.DMA((6,)),
            pltpu.SemaphoreType.DMA((5,)),
            pltpu.SemaphoreType.REGULAR,
            pltpu.SemaphoreType.REGULAR,
        ],
        compiler_params=pltpu.CompilerParams(
            collective_id=0,
            disable_semaphore_checks=True,
            disable_bounds_checks=True,
        ),
    )(x.T)
    return out_t.T
```

```python
import jax
import jax.numpy as jnp
from jax import lax
from jax.experimental import pallas as pl
from jax.experimental.pallas import tpu as pltpu

BF16 = jnp.bfloat16
F32 = jnp.float32
MESH = pl.DeviceIdType.MESH
NT = (((1,), (1,)), ((), ()))

A, B, D, C = 0, 1, 2, 3


class _Lay:
    def __init__(self, slot, sub):
        self.slot, self.sub = list(slot), dict(sub)

    def copy(self):
        return _Lay(self.slot, self.sub)

    def dist(self, bit):
        return [d for d, b in self.sub.items() if b == bit][0]


def _oe_merge(lo, n, r=1):
    m = 2 * r
    if m < n:
        yield from _oe_merge(lo, n, m)
        yield from _oe_merge(lo + r, n, m)
        for i in range(lo + r, lo + n - r, m):
            yield (i, i + r)
    else:
        yield (lo, lo + r)


def _oe_sort(lo, n):
    if n > 1:
        yield from _oe_sort(lo, n // 2)
        yield from _oe_sort(lo + n // 2, n // 2)
        yield from _oe_merge(lo, n)


def _network(tiles, net):
    t = list(tiles)
    for i, j in net:
        t[i], t[j] = jnp.minimum(t[i], t[j]), jnp.maximum(t[i], t[j])
    return t


def _cat(parts):
    return jnp.concatenate(parts, axis=0)


def _split(v, lay, bit):
    k = lay.slot.index(bit)
    lay.slot.append(lay.slot.pop(k))
    h, w = v.shape[0] // 2, v.shape[-1]
    if 1 << k == h:
        return v[:h], v[h:]
    v5 = v.reshape(h >> k, 2, 1 << k, 8, w)
    return v5[:, 0].reshape(h, 8, w), v5[:, 1].reshape(h, 8, w)


def _sub_mask(d, shape):
    return (lax.broadcasted_iota(jnp.int32, shape, 1) & d) != 0


def _cmp(v, lay, bit, desc=False):
    a, b = _split(v, lay, bit)
    lo, hi = jnp.minimum(a, b), jnp.maximum(a, b)
    return _cat([hi, lo] if desc else [lo, hi])


def _cmp_sub(v, lay, bit):
    d = lay.dist(bit)
    up = pltpu.roll(v, d, 1)
    dn = up if d == 4 else pltpu.roll(v, 8 - d, 1)
    return jnp.where(_sub_mask(d, v.shape), jnp.maximum(v, up), jnp.minimum(v, dn))


def _swap(v, lay, bit_in, bit_out, mirror=False, negate=False):
    d = lay.dist(bit_in)
    a, b = _split(v, lay, bit_out)
    m = _sub_mask(d, a.shape)
    a2 = jnp.where(m, pltpu.roll(b, d, 1), a)
    if mirror:
        b2 = jnp.where(m, a, pltpu.roll(b, 8 - d, 1))
    else:
        b2 = jnp.where(m, b, pltpu.roll(a, 8 - d, 1))
    lay.slot[-1], lay.sub[d] = bit_in, bit_out
    return _cat([a2, -b2 if negate else b2])


def _tiles(v, lay, slot):
    pos = [lay.slot.index(b) for b in slot]
    idx = [sum(((j >> k) & 1) << p for k, p in enumerate(pos)) for j in range(len(v))]
    lay.slot = list(slot)
    return [v[i:i + 1] for i in idx]


def _merge_tiles(v, lay, rev):
    t, h = _tiles(v, lay, sorted(lay.slot)), len(v) // 2
    return _network(t[:h] + (t[:h - 1:-1] if rev else t[h:]), _oe_merge(0, 2 * h))


def _presort(v):
    n = len(v)
    nb = n.bit_length() - 1
    lay = _Lay(range(nb), {2: nb, 1: nb + 1, 4: nb + 2})
    arrive = [q * (n // 4) + j for j in range(n // 4) for q in range(4)]
    v = _cat(_network([v[a:a + 1] for a in arrive], _oe_sort(0, n)))
    v = _swap(v, lay, nb, 0, mirror=True)
    v = _cat(_merge_tiles(v, lay, False))
    v = _cmp(_swap(v, lay, 0, 1), lay, 0)
    v = _swap(v, lay, nb + 1, 0, negate=True)
    v = _cat(_merge_tiles(v, lay, True))
    v = _cmp(_swap(v, lay, 1, 2), lay, 1)
    v = _cmp(_swap(v, lay, 0, 1), lay, 0)
    v = _swap(v, lay, nb + 2, 0, negate=True)
    return _merge_tiles(v, lay, True), lay


LAY_LIST = _Lay([4, 5, 6, 0], {2: 3, 1: 2, 4: 1})


def _finish(pre, desc):
    tiles, lay = pre[0], pre[1].copy()
    v = _cat(tiles[::-1] if desc else tiles)
    for b in (2, 1, 0):
        v = _cmp(_swap(v, lay, b, b + 1), lay, b, desc)
    assert lay.slot in ([4, 5, 0], LAY_LIST.slot) and lay.sub == LAY_LIST.sub
    return v


def _fold64(t, h):
    w = t.shape[-1]
    t5 = t.reshape(2, 2, 4, 8, w)
    up = jnp.minimum(t5[:, 1], h.reshape(2, 4, 8, w))
    return jnp.concatenate([t5[:, 0], up], axis=1).reshape(16, 8, w)


def _bitonic_to_list(v):
    lay = LAY_LIST.copy()
    for b in (6, 5, 4):
        v = _cmp(v, lay, b)
    for b in (3, 2, 1):
        v = _cmp_sub(v, lay, b)
    v = _cmp(v, lay, 0)
    return _cat(_tiles(v, lay, LAY_LIST.slot))


def _bitonic_to_rows(v):
    lay = LAY_LIST.copy()
    for b in (6, 5, 4):
        v = _cmp(v, lay, b)
    for b, e in ((3, 0), (2, 3), (1, 2), (0, 1)):
        v = _cmp(_swap(v, lay, b, e), lay, b)
    v = _swap(v, lay, 3, 0)
    assert lay.sub == {4: 2, 2: 1, 1: 0}
    return _cat(_tiles(v, lay, [3, 4, 5, 6])).reshape(128, v.shape[-1])


def _to_lanes(w, rows=128):
    w, parts = w.astype(BF16), []
    for q in range(4):
        r = lax.broadcasted_iota(jnp.int32, (rows // 4, 128), 0) + rows // 4 * q
        c = lax.broadcasted_iota(jnp.int32, (rows // 4, 128), 1) & (rows - 1)
        sign = jnp.where(((r ^ (r >> 2)) & 1) == 1, -1.0, 1.0)
        sel = jnp.where(r == c, sign, 0.0).astype(BF16)
        parts.append(lax.dot_general(sel, w, NT, preferred_element_type=F32))
    return _cat(parts).reshape(rows // 8, 8, w.shape[0])


MXU_RANKS = 48


def _write_out(rows, o_ref):
    y = rows[:, :64]
    hi = _cat([jnp.zeros((MXU_RANKS, 64), F32), y[MXU_RANKS:]]).T
    o_ref[:, MXU_RANKS:] = hi[:, MXU_RANKS:]
    lo = y[:MXU_RANKS].astype(BF16)
    for q in range(4):
        r = lax.broadcasted_iota(jnp.int32, (16, 64), 0) + 16 * q
        c = lax.broadcasted_iota(jnp.int32, (16, 64), 1)
        o_ref[16 * q:16 * (q + 1), :MXU_RANKS] = lax.dot_general(
            (r == c).astype(BF16), lo, NT, preferred_element_type=F32)


def _left(shape):
    return lax.broadcasted_iota(jnp.int32, shape, len(shape) - 1) < 64


def _mix(p, q, left=None):
    return jnp.where(_left(p.shape) if left is None else left, p, q).astype(BF16)


def _unmix(h):
    h = h.astype(F32)
    return [jnp.where(_left(h.shape), h, 0.0), jnp.where(_left(h.shape), 0.0, h)]


ORDER = {A: (B, C, D), B: (A, D, C), C: (A, D, B), D: (A, B, C)}


def _body(x_ref, o_ref, xin, lst, rlst, first, rb_raw, rd_r1, rd_r2,
          s1a, s1b, s2a, s2b, r1a, r1b, r2a, r2b, lsem, ssem, rsem, psem, dsem):
    def load(r0, n, k):
        return pltpu.make_async_copy(
            x_ref.at[pl.ds(r0, n)], xin.at[pl.ds(r0, n)], lsem.at[k])

    ld_a, ld_b = load(0, 8, 0), load(16, 32, 1)
    ld_c, ld_d = load(8, 8, 2), load(48, 16, 3)
    me = lax.axis_index("i")
    ld_a.start()
    ld_b.start()
    bar = pltpu.get_barrier_semaphore()

    def sig(sem, dev):
        pl.semaphore_signal(sem, inc=1, device_id=(dev,), device_id_type=MESH)

    def rdma(src, dst, s, r, dev):
        return pltpu.make_async_remote_copy(
            src_ref=src, dst_ref=dst, send_sem=ssem.at[s], recv_sem=rsem.at[r],
            device_id=(dev,), device_id_type=MESH)

    def send(src, dst):
        slot = ORDER[dst].index(src)
        return rdma(lst, rlst.at[slot], dst, slot, dst)

    b_raw = lambda: rdma(x_ref, rb_raw, A, 0, A)
    d_r1 = lambda: rdma(x_ref.at[pl.ds(48, 16)], rd_r1, A, 2, A)
    d_r2 = lambda: rdma(x_ref.at[pl.ds(8, 8)], rd_r2, 4, 3, A)
    d_1a = lambda: rdma(s1a, r1a, 5, 4, A)
    d_1b = lambda: rdma(s1b, r1b, 6, 5, A)
    d_2a = lambda: rdma(s2a, r2a, 7, 6, A)
    d_2b = lambda: rdma(s2b, r2b, 8, 7, A)

    @pl.when(me == D)
    def _():
        pl.semaphore_wait(bar, 1)
        d_r1().start()
        d_r2().start()
        sig(dsem, A)
        left4 = _left((4, 128))
        ld_a.wait()
        s1a[...] = _mix(xin[0:4, :], xin[4:8, :], left4)
        d_1a().start()
        ld_b.wait()
        s1b[...] = _mix(xin[16:32, :], xin[32:48, :])
        d_1b().start()
        s2a[...] = _mix(xin[4:8, :], xin[0:4, :])
        s2b[...] = _mix(xin[32:48, :], xin[16:32, :])
        d_2a().start()
        d_2b().start()
        ld_c.start()
        ld_d.start()

    @pl.when(me != D)
    def _():
        ld_c.start()
        ld_d.start()

        @pl.when(me == A)
        def _():
            sig(bar, D)
            sig(bar, B)
            sig(bar, C)

        @pl.when(me != A)
        def _():
            sig(bar, A)
            pl.semaphore_wait(bar, 1)

        @pl.when(me == B)
        def _():
            b_raw().start()

        ld_a.wait()
        ld_b.wait()

    ld_c.wait()
    ld_d.wait()

    def presort_dup(w):
        return _presort(_to_lanes(_cat([w, w])))

    pre = presort_dup(xin[...])
    dn = _finish(pre, True).reshape(128, 128)
    lst[...] = _mix(dn[:64], dn[64:])

    for X, Y in ((B, C), (C, B)):
        @pl.when(me == X)
        def _(X=X, Y=Y):
            if X == C:
                send(C, A).start()
            pl.semaphore_wait(psem, 1)
            send(X, Y).start()

    @pl.when(me == D)
    def _():
        pl.semaphore_wait(bar, 1)
        sig(dsem, B)
        sig(dsem, C)
        send(D, B).start()
        send(D, C).start()

    own = _finish(pre, False)

    def get(slot, both):
        rdma(lst, rlst.at[slot], 0, slot, A).wait_recv()
        p = rlst[slot].astype(F32)
        q = pltpu.roll(p, 64, 1)
        if both:
            left = _left(p.shape)
            p, q = jnp.where(left, p, q), jnp.where(left, q, p)
        return _cat([p, q]).reshape(16, 8, 128)

    def swap_halves(v):
        return pltpu.roll(v.reshape(128, 128), 64, 1).reshape(16, 8, 128)

    @pl.when(me == A)
    def _():
        pl.semaphore_wait(bar, 2)
        sig(bar, D)
        sig(psem, B)
        sig(psem, C)
        send(A, B).start()
        send(A, C).start()
        pl.semaphore_wait(dsem, 1)
        send(A, D).start()
        b_raw().wait_recv()
        first[...] = _finish(presort_dup(rb_raw[...]), True)

    @pl.when(me != A)
    def _():
        first[...] = get(0, True)

    l1 = first[...]
    left = _left(l1.shape)
    lh = _bitonic_to_list(jnp.where(left, jnp.minimum(own, l1), jnp.maximum(own, l1)))

    for X in (B, C):
        @pl.when(me == X)
        def _(X=X):
            pl.semaphore_wait(dsem, 1)
            send(X, D).start()

    l2 = get(1, True)
    hl = swap_halves(lh)
    low = me < 2
    inf = jnp.float32(jnp.inf)
    lo2 = jnp.where(low, jnp.where(left, -inf, hl), lh)
    hi2 = jnp.where(low, lh, jnp.where(left, hl, inf))
    uv = _bitonic_to_list(jnp.minimum(jnp.maximum(l2, lo2), hi2))

    @pl.when(me != A)
    def _():
        l3 = get(2, False)
        vu = swap_halves(uv)
        lo3 = jnp.where(me == C, vu, uv)
        hi3 = jnp.where(me == C, inf, vu)
        _write_out(_bitonic_to_rows(jnp.minimum(jnp.maximum(l3, lo3), hi3)), o_ref)
        for X, dsts, raws in ((B, (C, D), (b_raw,)), (C, (A, B, D), ()),
                              (D, (B, C), (d_r1, d_r2, d_1a, d_1b, d_2a, d_2b))):
            @pl.when(me == X)
            def _(X=X, dsts=dsts, raws=raws):
                for dst in dsts:
                    send(X, dst).wait_send()
                for raw in raws:
                    raw().wait_send()

    @pl.when(me == A)
    def _():
        d_r1().wait_recv()
        g = _to_lanes(_cat([jnp.zeros((48, 128), F32), rd_r1[...]]))[:, :, 48:64]
        for dst in (B, C, D):
            send(A, dst).wait_send()
        d_r2().wait_recv()
        r2 = _unmix(rd_r2[...])
        d_1a().wait_recv()
        d_1b().wait_recv()
        w = _cat(_unmix(r1a[...]) + r2[:1] + _unmix(r1b[...]))
        p1 = jnp.concatenate([_to_lanes(w, 64), g[:8]], axis=2)
        d_2a().wait_recv()
        d_2b().wait_recv()
        t = _bitonic_to_list(_fold64(uv[:, :, :64], _finish(_presort(p1), True)))
        w = _cat(_unmix(r2a[...])[::-1] + r2[1:] + _unmix(r2b[...])[::-1])
        p2 = jnp.concatenate([_to_lanes(w, 64), g[8:]], axis=2)
        p2 = jnp.where(_left(p2.shape), p2, t[:8])
        _write_out(_bitonic_to_rows(_fold64(t, _finish(_presort(p2), True))), o_ref)


def pallas_dist_sort_i_m128_n64_kernel(x: jax.Array):
    batch = [pltpu.VMEM((4, 128), BF16), pltpu.VMEM((16, 128), BF16)]
    out_t = pl.pallas_call(
        _body,
        out_shape=jax.ShapeDtypeStruct((64, 128), x.dtype),
        in_specs=[pl.BlockSpec(memory_space=pl.ANY)],
        out_specs=pl.BlockSpec(memory_space=pltpu.VMEM),
        scratch_shapes=[
            pltpu.VMEM((64, 128), F32),
            pltpu.VMEM((64, 128), BF16),
            pltpu.VMEM((3, 64, 128), BF16),
            pltpu.VMEM((16, 8, 128), F32),
            pltpu.VMEM((64, 128), F32),
            pltpu.VMEM((16, 128), F32),
            pltpu.VMEM((8, 128), F32),
            *(batch * 4),
            pltpu.SemaphoreType.DMA((4,)),
            pltpu.SemaphoreType.DMA((9,)),
            pltpu.SemaphoreType.DMA((8,)),
            pltpu.SemaphoreType.REGULAR,
            pltpu.SemaphoreType.REGULAR,
        ],
        compiler_params=pltpu.CompilerParams(
            collective_id=0,
            disable_semaphore_checks=True,
            disable_bounds_checks=True,
        ),
    )(x.T)
    return out_t.T
```

```python
import jax
import jax.numpy as jnp
from jax import lax
from jax.experimental import pallas as pl
from jax.experimental.pallas import tpu as pltpu

BF16 = jnp.bfloat16
F32 = jnp.float32
MESH = pl.DeviceIdType.MESH
NT = (((1,), (1,)), ((), ()))

A, B, D, C = 0, 1, 2, 3


class _Lay:
    def __init__(self, slot, sub):
        self.slot, self.sub = list(slot), dict(sub)

    def copy(self):
        return _Lay(self.slot, self.sub)

    def dist(self, bit):
        return [d for d, b in self.sub.items() if b == bit][0]


def _oe_merge(lo, n, r=1):
    m = 2 * r
    if m < n:
        yield from _oe_merge(lo, n, m)
        yield from _oe_merge(lo + r, n, m)
        for i in range(lo + r, lo + n - r, m):
            yield (i, i + r)
    else:
        yield (lo, lo + r)


def _oe_sort(lo, n):
    if n > 1:
        yield from _oe_sort(lo, n // 2)
        yield from _oe_sort(lo + n // 2, n // 2)
        yield from _oe_merge(lo, n)


def _network(tiles, net):
    t = list(tiles)
    for i, j in net:
        t[i], t[j] = jnp.minimum(t[i], t[j]), jnp.maximum(t[i], t[j])
    return t


def _cat(parts):
    return jnp.concatenate(parts, axis=0)


def _split(v, lay, bit):
    k = lay.slot.index(bit)
    lay.slot.append(lay.slot.pop(k))
    h, w = v.shape[0] // 2, v.shape[-1]
    if 1 << k == h:
        return v[:h], v[h:]
    v5 = v.reshape(h >> k, 2, 1 << k, 8, w)
    return v5[:, 0].reshape(h, 8, w), v5[:, 1].reshape(h, 8, w)


def _sub_mask(d, shape):
    return (lax.broadcasted_iota(jnp.int32, shape, 1) & d) != 0


def _cmp(v, lay, bit, desc=False):
    a, b = _split(v, lay, bit)
    lo, hi = jnp.minimum(a, b), jnp.maximum(a, b)
    return _cat([hi, lo] if desc else [lo, hi])


def _cmp_sub(v, lay, bit):
    d = lay.dist(bit)
    up = pltpu.roll(v, d, 1)
    dn = up if d == 4 else pltpu.roll(v, 8 - d, 1)
    return jnp.where(_sub_mask(d, v.shape), jnp.maximum(v, up), jnp.minimum(v, dn))


def _swap(v, lay, bit_in, bit_out, mirror=False, negate=False):
    d = lay.dist(bit_in)
    a, b = _split(v, lay, bit_out)
    m = _sub_mask(d, a.shape)
    a2 = jnp.where(m, pltpu.roll(b, d, 1), a)
    if mirror:
        b2 = jnp.where(m, a, pltpu.roll(b, 8 - d, 1))
    else:
        b2 = jnp.where(m, b, pltpu.roll(a, 8 - d, 1))
    lay.slot[-1], lay.sub[d] = bit_in, bit_out
    return _cat([a2, -b2 if negate else b2])


def _tiles(v, lay, slot):
    pos = [lay.slot.index(b) for b in slot]
    idx = [sum(((j >> k) & 1) << p for k, p in enumerate(pos)) for j in range(len(v))]
    lay.slot = list(slot)
    return [v[i:i + 1] for i in idx]


def _merge_tiles(v, lay, rev):
    t, h = _tiles(v, lay, sorted(lay.slot)), len(v) // 2
    return _network(t[:h] + (t[:h - 1:-1] if rev else t[h:]), _oe_merge(0, 2 * h))


def _presort(v):
    n = len(v)
    nb = n.bit_length() - 1
    lay = _Lay(range(nb), {2: nb, 1: nb + 1, 4: nb + 2})
    arrive = [q * (n // 4) + j for j in range(n // 4) for q in range(4)]
    v = _cat(_network([v[a:a + 1] for a in arrive], _oe_sort(0, n)))
    v = _swap(v, lay, nb, 0, mirror=True)
    v = _cat(_merge_tiles(v, lay, False))
    v = _cmp(_swap(v, lay, 0, 1), lay, 0)
    v = _swap(v, lay, nb + 1, 0, negate=True)
    v = _cat(_merge_tiles(v, lay, True))
    v = _cmp(_swap(v, lay, 1, 2), lay, 1)
    v = _cmp(_swap(v, lay, 0, 1), lay, 0)
    v = _swap(v, lay, nb + 2, 0, negate=True)
    return _merge_tiles(v, lay, True), lay


LAY_LIST = _Lay([4, 5, 6, 0], {2: 3, 1: 2, 4: 1})


def _finish(pre, desc):
    tiles, lay = pre[0], pre[1].copy()
    v = _cat(tiles[::-1] if desc else tiles)
    for b in (2, 1, 0):
        v = _cmp(_swap(v, lay, b, b + 1), lay, b, desc)
    assert lay.slot in ([4, 5, 0], LAY_LIST.slot) and lay.sub == LAY_LIST.sub
    return v


def _fold64(t, h):
    w = t.shape[-1]
    t5 = t.reshape(2, 2, 4, 8, w)
    up = jnp.minimum(t5[:, 1], h.reshape(2, 4, 8, w))
    return jnp.concatenate([t5[:, 0], up], axis=1).reshape(16, 8, w)


def _bitonic_to_list(v):
    lay = LAY_LIST.copy()
    for b in (6, 5, 4):
        v = _cmp(v, lay, b)
    for b in (3, 2, 1):
        v = _cmp_sub(v, lay, b)
    v = _cmp(v, lay, 0)
    return _cat(_tiles(v, lay, LAY_LIST.slot))


def _bitonic_to_rows(v):
    lay = LAY_LIST.copy()
    for b in (6, 5, 4):
        v = _cmp(v, lay, b)
    for b, e in ((3, 0), (2, 3), (1, 2), (0, 1)):
        v = _cmp(_swap(v, lay, b, e), lay, b)
    v = _swap(v, lay, 3, 0)
    assert lay.sub == {4: 2, 2: 1, 1: 0}
    return _cat(_tiles(v, lay, [3, 4, 5, 6])).reshape(128, v.shape[-1])


def _to_lanes(w, rows=128):
    w, parts = w.astype(BF16), []
    for q in range(4):
        r = lax.broadcasted_iota(jnp.int32, (rows // 4, 128), 0) + rows // 4 * q
        c = lax.broadcasted_iota(jnp.int32, (rows // 4, 128), 1) & (rows - 1)
        sign = jnp.where(((r ^ (r >> 2)) & 1) == 1, -1.0, 1.0)
        sel = jnp.where(r == c, sign, 0.0).astype(BF16)
        parts.append(lax.dot_general(sel, w, NT, preferred_element_type=F32))
    return _cat(parts).reshape(rows // 8, 8, w.shape[0])


MXU_RANKS = 48


def _write_out(rows, o_ref):
    y = rows[:, :64]
    hi = _cat([jnp.zeros((MXU_RANKS, 64), F32), y[MXU_RANKS:]]).T
    o_ref[:, MXU_RANKS:] = hi[:, MXU_RANKS:]
    lo = y[:MXU_RANKS].astype(BF16)
    for q in range(4):
        r = lax.broadcasted_iota(jnp.int32, (16, 64), 0) + 16 * q
        c = lax.broadcasted_iota(jnp.int32, (16, 64), 1)
        o_ref[16 * q:16 * (q + 1), :MXU_RANKS] = lax.dot_general(
            (r == c).astype(BF16), lo, NT, preferred_element_type=F32)


def _left(shape):
    return lax.broadcasted_iota(jnp.int32, shape, len(shape) - 1) < 64


def _mix(p, q, left=None):
    return jnp.where(_left(p.shape) if left is None else left, p, q).astype(BF16)


def _unmix(h):
    h = h.astype(F32)
    return [jnp.where(_left(h.shape), h, 0.0), jnp.where(_left(h.shape), 0.0, h)]


ORDER = {A: (B, C, D), B: (A, D, C), C: (A, D, B), D: (A, B, C)}


def _body(x_ref, o_ref, xin, lst, rlst, first, rb_raw, rd_r1, rd_r2,
          s1a, s1b, s2a, s2b, r1a, r1b, r2a, r2b, lsem, ssem, rsem, psem, dsem):
    def load(r0, n, k):
        return pltpu.make_async_copy(
            x_ref.at[pl.ds(r0, n)], xin.at[pl.ds(r0, n)], lsem.at[k])

    ld_a, ld_b = load(0, 8, 0), load(16, 32, 1)
    ld_c, ld_d = load(8, 8, 2), load(48, 16, 3)
    me = lax.axis_index("i")
    ld_a.start()
    ld_b.start()
    bar = pltpu.get_barrier_semaphore()

    def sig(sem, dev):
        pl.semaphore_signal(sem, inc=1, device_id=(dev,), device_id_type=MESH)

    def rdma(src, dst, s, r, dev):
        return pltpu.make_async_remote_copy(
            src_ref=src, dst_ref=dst, send_sem=ssem.at[s], recv_sem=rsem.at[r],
            device_id=(dev,), device_id_type=MESH)

    def send(src, dst):
        slot = ORDER[dst].index(src)
        return rdma(lst, rlst.at[slot], dst, slot, dst)

    b_raw = lambda: rdma(x_ref, rb_raw, A, 0, A)
    d_r1 = lambda: rdma(x_ref.at[pl.ds(48, 16)], rd_r1, A, 2, A)
    d_r2 = lambda: rdma(x_ref.at[pl.ds(8, 8)], rd_r2, 4, 3, A)
    d_1a = lambda: rdma(s1a, r1a, 5, 4, A)
    d_1b = lambda: rdma(s1b, r1b, 6, 5, A)
    d_2a = lambda: rdma(s2a, r2a, 7, 6, A)
    d_2b = lambda: rdma(s2b, r2b, 8, 7, A)

    @pl.when(me == D)
    def _():
        pl.semaphore_wait(bar, 1)
        d_r1().start()
        d_r2().start()
        sig(dsem, A)
        left4 = _left((4, 128))
        ld_a.wait()
        s1a[...] = _mix(xin[0:4, :], xin[4:8, :], left4)
        d_1a().start()
        ld_b.wait()
        s1b[...] = _mix(xin[16:32, :], xin[32:48, :])
        d_1b().start()
        s2a[...] = _mix(xin[4:8, :], xin[0:4, :])
        s2b[...] = _mix(xin[32:48, :], xin[16:32, :])
        d_2a().start()
        d_2b().start()
        ld_c.start()
        ld_d.start()

    @pl.when(me != D)
    def _():
        ld_c.start()
        ld_d.start()

        @pl.when(me == A)
        def _():
            sig(bar, D)
            sig(bar, B)
            sig(bar, C)

        @pl.when(me != A)
        def _():
            sig(bar, A)
            pl.semaphore_wait(bar, 1)

        @pl.when(me == B)
        def _():
            b_raw().start()

        ld_a.wait()
        ld_b.wait()

    ld_c.wait()
    ld_d.wait()

    def presort_dup(w):
        return _presort(_to_lanes(_cat([w, w])))

    pre = presort_dup(xin[...])
    dn = _finish(pre, True).reshape(128, 128)
    lst[...] = _mix(dn[:64], dn[64:])

    for X, Y in ((B, C), (C, B)):
        @pl.when(me == X)
        def _(X=X, Y=Y):
            if X == C:
                send(C, A).start()
            pl.semaphore_wait(psem, 1)
            send(X, Y).start()

    @pl.when(me == D)
    def _():
        pl.semaphore_wait(bar, 1)
        sig(dsem, B)
        sig(dsem, C)
        send(D, B).start()
        send(D, C).start()

    own = _finish(pre, False)

    def get(slot, both):
        rdma(lst, rlst.at[slot], 0, slot, A).wait_recv()
        p = rlst[slot].astype(F32)
        q = pltpu.roll(p, 64, 1)
        if both:
            left = _left(p.shape)
            p, q = jnp.where(left, p, q), jnp.where(left, q, p)
        return _cat([p, q]).reshape(16, 8, 128)

    def swap_halves(v):
        return pltpu.roll(v.reshape(128, 128), 64, 1).reshape(16, 8, 128)

    @pl.when(me == A)
    def _():
        pl.semaphore_wait(bar, 2)
        sig(bar, D)
        sig(psem, B)
        sig(psem, C)
        send(A, B).start()
        send(A, C).start()
        pl.semaphore_wait(dsem, 1)
        send(A, D).start()
        b_raw().wait_recv()
        first[...] = _finish(presort_dup(rb_raw[...]), True)

    @pl.when(me != A)
    def _():
        first[...] = get(0, True)

    l1 = first[...]
    left = _left(l1.shape)
    lh = _bitonic_to_list(jnp.where(left, jnp.minimum(own, l1), jnp.maximum(own, l1)))

    for X in (B, C):
        @pl.when(me == X)
        def _(X=X):
            pl.semaphore_wait(dsem, 1)
            send(X, D).start()

    l2 = get(1, True)
    hl = swap_halves(lh)
    low = me < 2
    inf = jnp.float32(jnp.inf)
    lo2 = jnp.where(low, jnp.where(left, -inf, hl), lh)
    hi2 = jnp.where(low, lh, jnp.where(left, hl, inf))
    uv = _bitonic_to_list(jnp.minimum(jnp.maximum(l2, lo2), hi2))

    @pl.when(me != A)
    def _():
        l3 = get(2, False)
        vu = swap_halves(uv)
        lo3 = jnp.where(me == C, vu, uv)
        hi3 = jnp.where(me == C, inf, vu)
        _write_out(_bitonic_to_rows(jnp.minimum(jnp.maximum(l3, lo3), hi3)), o_ref)
        for X, dsts, raws in ((B, (C, D), (b_raw,)), (C, (A, B, D), ()),
                              (D, (B, C), (d_r1, d_r2, d_1a, d_1b, d_2a, d_2b))):
            @pl.when(me == X)
            def _(X=X, dsts=dsts, raws=raws):
                for dst in dsts:
                    send(X, dst).wait_send()
                for raw in raws:
                    raw().wait_send()

    @pl.when(me == A)
    def _():
        d_r1().wait_recv()
        g = _to_lanes(_cat([jnp.zeros((48, 128), F32), rd_r1[...]]))[:, :, 48:64]
        for dst in (B, C, D):
            send(A, dst).wait_send()
        d_r2().wait_recv()
        r2 = _unmix(rd_r2[...])
        d_1a().wait_recv()
        d_1b().wait_recv()
        w = _cat(_unmix(r1a[...]) + r2[:1] + _unmix(r1b[...]))
        p1 = jnp.concatenate([_to_lanes(w, 64), g[:8]], axis=2)
        d_2a().wait_recv()
        d_2b().wait_recv()
        t = _bitonic_to_list(_fold64(uv[:, :, :64], _finish(_presort(p1), True)))
        w = _cat(_unmix(r2a[...])[::-1] + r2[1:] + _unmix(r2b[...])[::-1])
        p2 = jnp.concatenate([_to_lanes(w, 64), g[8:]], axis=2)
        p2 = jnp.where(_left(p2.shape), p2, t[:8])
        _write_out(_bitonic_to_rows(_fold64(t, _finish(_presort(p2), True))), o_ref)


def pallas_dist_sort_i_m128_n64_kernel(x: jax.Array):
    batch = [pltpu.VMEM((4, 128), BF16), pltpu.VMEM((16, 128), BF16)]
    out_t = pl.pallas_call(
        _body,
        out_shape=jax.ShapeDtypeStruct((64, 128), x.dtype),
        in_specs=[pl.BlockSpec(memory_space=pl.ANY)],
        out_specs=pl.BlockSpec(memory_space=pltpu.VMEM),
        scratch_shapes=[
            pltpu.VMEM((64, 128), F32),
            pltpu.VMEM((64, 128), BF16),
            pltpu.VMEM((3, 64, 128), BF16),
            pltpu.VMEM((16, 8, 128), F32),
            pltpu.VMEM((64, 128), F32),
            pltpu.VMEM((16, 128), F32),
            pltpu.VMEM((8, 128), F32),
            *(batch * 4),
            pltpu.SemaphoreType.DMA((4,)),
            pltpu.SemaphoreType.DMA((9,)),
            pltpu.SemaphoreType.DMA((8,)),
            pltpu.SemaphoreType.REGULAR,
            pltpu.SemaphoreType.REGULAR,
        ],
        compiler_params=pltpu.CompilerParams(
            collective_id=0, disable_semaphore_checks=True),
    )(x.T)
    return out_t.T
```
